```python
import numpy as np

kernel_name = "dist_rope_attn_htp_bs_b2_sq512_d1024_hq8_dh128"

def setup_inputs():
    x = np.random.randn(8, 512, 1024).astype(np.float32)
    Wq = np.random.randn(1024, 4096).astype(np.float32) * 0.02
    Wk = np.random.randn(1024, 4096).astype(np.float32) * 0.02
    Wv = np.random.randn(1024, 4096).astype(np.float32) * 0.02
    Wo = np.random.randn(4096, 1024).astype(np.float32) * 0.02
    return {"x": x, "Wq": Wq, "Wk": Wk, "Wv": Wv, "Wo": Wo}

def reference(x, Wq, Wk, Wv, Wo):
    B, Sq, Hq, Dh = 8, 512, 32, 128
    inv = 1.0 / (10000.0 ** (np.arange(0, Dh, 2) / Dh))
    pos = np.arange(Sq)[:, None] * inv[None, :]
    cos = np.repeat(np.cos(pos), 2, axis=-1).astype(np.float32)
    sin = np.repeat(np.sin(pos), 2, axis=-1).astype(np.float32)
    def rot(t):
        t2 = t.reshape(B, Sq, Hq, Dh // 2, 2)
        t_r = np.stack([-t2[..., 1], t2[..., 0]], axis=-1).reshape(B, Sq, Hq, Dh)
        return t * cos[None, :, None, :] + t_r * sin[None, :, None, :]
    Q = rot((x @ Wq).reshape(B, Sq, Hq, Dh))
    K = rot((x @ Wk).reshape(B, Sq, Hq, Dh))
    V = (x @ Wv).reshape(B, Sq, Hq, Dh)
    s = np.einsum('bihd,bjhd->bhij', Q, K).astype(np.float32) * 0.08838834764831843
    s_max = s.max(axis=-1, keepdims=True)
    w = np.exp(s - s_max)
    w = w / w.sum(axis=-1, keepdims=True)
    ctx = np.einsum('bhij,bjhd->bihd', w, V).reshape(B, Sq, Hq * Dh)
    return ctx @ Wo
```

```python
import numpy as np

import jax
import jax.numpy as jnp
from jax import lax
from jax.experimental import pallas as pl
from jax.experimental.pallas import tpu as pltpu

N_DEV = 4
B_LOC = 2
SQ = 512
D = 1024
H_LOC = 8
DH = 128
N_UNITS = N_DEV * B_LOC
SCALE = 0.08838834764831843


def _rope_tables():
    inv = 1.0 / (10000.0 ** (np.arange(0, DH, 2) / DH))
    pos = np.arange(SQ)[:, None] * inv[None, :]
    cos = np.repeat(np.cos(pos), 2, axis=-1).astype(np.float32)
    sin = np.repeat(np.sin(pos), 2, axis=-1).astype(np.float32)
    sign = np.where(np.arange(DH) % 2 == 0, -1.0, 1.0).astype(np.float32)
    return cos, sin * sign[None, :]


def pallas_dist_rope_attn_htp_bs_b2_sq512_d1024_hq8_dh128_kernel(
    x: jax.Array,
    Wq: jax.Array,
    Wk: jax.Array,
    Wv: jax.Array,
    Wo: jax.Array,
):
    cos_np, sin_np = _rope_tables()

    def body(x_hbm, wq_hbm, wk_hbm, wv_hbm, wo_hbm, cos_ref, sin_ref, out_ref,
             xf_ref, wf_ref, wqkv_ref, wo_ref, xg_ref, psend_ref, precv_ref,
             qkv_ref, ctx_ref,
             load_sems, xsend_sems, xrecv_sems, psend_sems, precv_sems):
        me = lax.axis_index("i")
        left = (me + N_DEV - 1) % N_DEV
        right = (me + 1) % N_DEV
        diag = (me + 2) % N_DEV

        x_load = pltpu.make_async_copy(x_hbm, xf_ref, load_sems.at[0])
        x_load.start()
        w_loads = []
        for i, w in enumerate((wq_hbm, wk_hbm, wv_hbm, wo_hbm)):
            cp = pltpu.make_async_copy(w, wf_ref.at[i], load_sems.at[1 + i])
            cp.start()
            w_loads.append(cp)

        x_load.wait()
        xg_ref[0] = xf_ref[0].astype(jnp.bfloat16)
        xg_ref[N_UNITS - 1] = xf_ref[1].astype(jnp.bfloat16)

        x_sends = [
            (0, 1, right), (0, 2, left),
            (N_UNITS - 1, 3, right), (N_UNITS - 1, 4, left),
            (0, 5, diag), (N_UNITS - 1, 6, diag),
        ]
        x_rdmas = []
        for i, (su, du, dev) in enumerate(x_sends):
            r = pltpu.make_async_remote_copy(
                src_ref=xg_ref.at[su], dst_ref=xg_ref.at[du],
                send_sem=xsend_sems.at[i], recv_sem=xrecv_sems.at[du],
                device_id=(dev,), device_id_type=pl.DeviceIdType.MESH)
            r.start()
            x_rdmas.append(r)

        for i in range(3):
            w_loads[i].wait()
            wqkv_ref[:, i * D:(i + 1) * D] = wf_ref[i].astype(jnp.bfloat16)
        w_loads[3].wait()
        wo_ref[...] = wf_ref[3].astype(jnp.bfloat16)

        lane = lax.broadcasted_iota(jnp.int32, (SQ, DH), 1)
        even = (lane % 2) == 0

        def unit(u, carry):
            is_remote = jnp.logical_and(u >= 1, u <= N_UNITS - 2)

            @pl.when(is_remote)
            def _():
                pltpu.make_async_remote_copy(
                    src_ref=xg_ref.at[u], dst_ref=xg_ref.at[u],
                    send_sem=xsend_sems.at[0], recv_sem=xrecv_sems.at[u],
                    device_id=(me,), device_id_type=pl.DeviceIdType.MESH,
                ).wait_recv()

            xu = xg_ref[u]
            qkv = jnp.dot(xu, wqkv_ref[...], preferred_element_type=jnp.float32)
            cos = cos_ref[...]
            sin = sin_ref[...]
            for c in range(2 * H_LOC):
                t = qkv[:, c * DH:(c + 1) * DH]
                tr = jnp.where(even, pltpu.roll(t, DH - 1, 1), pltpu.roll(t, 1, 1))
                r = t * cos + tr * sin
                if c < H_LOC:
                    r = r * SCALE
                qkv_ref[c] = r.astype(jnp.bfloat16)
            for c in range(2 * H_LOC, 3 * H_LOC):
                qkv_ref[c] = qkv[:, c * DH:(c + 1) * DH].astype(jnp.bfloat16)

            for h in range(H_LOC):
                q = qkv_ref[h]
                k = qkv_ref[H_LOC + h]
                v = qkv_ref[2 * H_LOC + h]
                s = lax.dot_general(q, k, (((1,), (1,)), ((), ())),
                                    preferred_element_type=jnp.float32)
                m = jnp.max(s, axis=-1, keepdims=True)
                p = jnp.exp(s - m)
                l = jnp.sum(p, axis=-1, keepdims=True)
                o = jnp.dot(p.astype(jnp.bfloat16), v,
                            preferred_element_type=jnp.float32)
                ctx_ref[:, h * DH:(h + 1) * DH] = (o / l).astype(jnp.bfloat16)

            part = jnp.dot(ctx_ref[...], wo_ref[...],
                           preferred_element_type=jnp.float32)

            @pl.when(u == 0)
            def _():
                out_ref[0] = part

            @pl.when(u == N_UNITS - 1)
            def _():
                out_ref[1] = part

            @pl.when(is_remote)
            def _():
                psend_ref[u] = part.astype(jnp.bfloat16)
                dev = jnp.where(u >= 5, diag, jnp.where(u % 2 == 1, left, right))
                pltpu.make_async_remote_copy(
                    src_ref=psend_ref.at[u], dst_ref=precv_ref.at[u],
                    send_sem=psend_sems.at[u], recv_sem=precv_sems.at[u],
                    device_id=(dev,), device_id_type=pl.DeviceIdType.MESH,
                ).start()

            return carry

        lax.fori_loop(0, N_UNITS, unit, 0)

        for r in x_rdmas:
            r.wait_send()
        for u in range(1, N_UNITS - 1):
            pltpu.make_async_remote_copy(
                src_ref=psend_ref.at[u], dst_ref=precv_ref.at[u],
                send_sem=psend_sems.at[u], recv_sem=precv_sems.at[u],
                device_id=(me,), device_id_type=pl.DeviceIdType.MESH,
            ).wait()

        out_ref[0] = (out_ref[0]
                      + precv_ref[1].astype(jnp.float32)
                      + precv_ref[2].astype(jnp.float32)
                      + precv_ref[5].astype(jnp.float32))
        out_ref[1] = (out_ref[1]
                      + precv_ref[3].astype(jnp.float32)
                      + precv_ref[4].astype(jnp.float32)
                      + precv_ref[6].astype(jnp.float32))

    out_shape = jax.ShapeDtypeStruct((B_LOC, SQ, D), jnp.float32)
    return pl.pallas_call(
        body,
        out_shape=out_shape,
        in_specs=[pl.BlockSpec(memory_space=pl.ANY)] * 5
        + [pl.BlockSpec(memory_space=pltpu.VMEM)] * 2,
        out_specs=pl.BlockSpec(memory_space=pltpu.VMEM),
        scratch_shapes=[
            pltpu.VMEM((B_LOC, SQ, D), jnp.float32),
            pltpu.VMEM((4, D, D), jnp.float32),
            pltpu.VMEM((D, 3 * D), jnp.bfloat16),
            pltpu.VMEM((D, D), jnp.bfloat16),
            pltpu.VMEM((N_UNITS, SQ, D), jnp.bfloat16),
            pltpu.VMEM((N_UNITS, SQ, D), jnp.bfloat16),
            pltpu.VMEM((N_UNITS, SQ, D), jnp.bfloat16),
            pltpu.VMEM((3 * H_LOC, SQ, DH), jnp.bfloat16),
            pltpu.VMEM((SQ, D), jnp.bfloat16),
            pltpu.SemaphoreType.DMA((5,)),
            pltpu.SemaphoreType.DMA((6,)),
            pltpu.SemaphoreType.DMA((N_UNITS,)),
            pltpu.SemaphoreType.DMA((N_UNITS,)),
            pltpu.SemaphoreType.DMA((N_UNITS,)),
        ],
        compiler_params=pltpu.CompilerParams(
            vmem_limit_bytes=100 * 1024 * 1024,
        ),
    )(x, Wq, Wk, Wv, Wo, jnp.asarray(cos_np), jnp.asarray(sin_np))
```

```python
import numpy as np

import jax
import jax.numpy as jnp
from jax import lax
from jax.experimental import pallas as pl
from jax.experimental.pallas import tpu as pltpu

N_DEV = 4
B_LOC = 2
SQ = 512
D = 1024
H_LOC = 8
DH = 128
N_UNITS = N_DEV * B_LOC
SCALE = 0.08838834764831843


def _rope_tables():
    inv = 1.0 / (10000.0 ** (np.arange(0, DH, 2) / DH))
    pos = np.arange(SQ)[:, None] * inv[None, :]
    cos = np.repeat(np.cos(pos), 2, axis=-1).astype(np.float32)
    sin = np.repeat(np.sin(pos), 2, axis=-1).astype(np.float32)
    sign = np.where(np.arange(DH) % 2 == 0, -1.0, 1.0).astype(np.float32)
    return cos, sin * sign[None, :]


def pallas_dist_rope_attn_htp_bs_b2_sq512_d1024_hq8_dh128_kernel(
    x: jax.Array,
    Wq: jax.Array,
    Wk: jax.Array,
    Wv: jax.Array,
    Wo: jax.Array,
):
    cos_np, sin_np = _rope_tables()

    def body(x_hbm, wq_hbm, wk_hbm, wv_hbm, wo_hbm, cos_ref, sin_ref, out_ref,
             xf_ref, wf_ref, wqkv_ref, wo_ref, xg_ref, psend_ref, precv_ref,
             qkv_ref, ctx_ref,
             load_sems, xsend_sems, xrecv_sems, psend_sems, precv_sems):
        me = lax.axis_index("i")
        left = (me + N_DEV - 1) % N_DEV
        right = (me + 1) % N_DEV
        diag = (me + 2) % N_DEV

        x_loads = []
        for b in range(B_LOC):
            cp = pltpu.make_async_copy(x_hbm.at[b], xf_ref.at[b], load_sems.at[b])
            cp.start()
            x_loads.append(cp)
        w_loads = []
        for i, w in enumerate((wq_hbm, wk_hbm, wv_hbm, wo_hbm)):
            cp = pltpu.make_async_copy(w, wf_ref.at[i], load_sems.at[2 + i])
            cp.start()
            w_loads.append(cp)

        x_loads[0].wait()
        xg_ref[0] = xf_ref[0].astype(jnp.bfloat16)
        x_loads[1].wait()
        xg_ref[N_UNITS - 1] = xf_ref[1].astype(jnp.bfloat16)

        x_sends = [
            (0, 1, right), (0, 2, left),
            (N_UNITS - 1, 3, right), (N_UNITS - 1, 4, left),
            (0, 5, diag), (N_UNITS - 1, 6, diag),
        ]
        x_rdmas = []
        for i, (su, du, dev) in enumerate(x_sends):
            r = pltpu.make_async_remote_copy(
                src_ref=xg_ref.at[su], dst_ref=xg_ref.at[du],
                send_sem=xsend_sems.at[i], recv_sem=xrecv_sems.at[du],
                device_id=(dev,), device_id_type=pl.DeviceIdType.MESH)
            r.start()
            x_rdmas.append(r)

        lane = lax.broadcasted_iota(jnp.int32, (SQ, DH), 1)
        even = (lane % 2) == 0

        def unit(u, carry):
            is_remote = jnp.logical_and(u >= 1, u <= N_UNITS - 2)

            @pl.when(is_remote)
            def _():
                pltpu.make_async_remote_copy(
                    src_ref=xg_ref.at[u], dst_ref=xg_ref.at[u],
                    send_sem=xsend_sems.at[0], recv_sem=xrecv_sems.at[u],
                    device_id=(me,), device_id_type=pl.DeviceIdType.MESH,
                ).wait_recv()

            xu = xg_ref[u]
            cos = cos_ref[...]
            sin = sin_ref[...]
            for i in range(3):
                @pl.when(u == 0)
                def _():
                    w_loads[i].wait()
                    wqkv_ref[i] = wf_ref[i].astype(jnp.bfloat16)

                y = jnp.dot(xu, wqkv_ref[i], preferred_element_type=jnp.float32)
                for c in range(H_LOC):
                    t = y[:, c * DH:(c + 1) * DH]
                    if i < 2:
                        tr = jnp.where(even, pltpu.roll(t, DH - 1, 1),
                                       pltpu.roll(t, 1, 1))
                        t = t * cos + tr * sin
                    if i == 0:
                        t = t * SCALE
                    qkv_ref[i * H_LOC + c] = t.astype(jnp.bfloat16)

            for h in range(H_LOC):
                q = qkv_ref[h]
                k = qkv_ref[H_LOC + h]
                v = qkv_ref[2 * H_LOC + h]
                s = lax.dot_general(q, k, (((1,), (1,)), ((), ())),
                                    preferred_element_type=jnp.float32)
                m = jnp.max(s, axis=-1, keepdims=True)
                p = jnp.exp(s - m)
                l = jnp.sum(p, axis=-1, keepdims=True)
                o = jnp.dot(p.astype(jnp.bfloat16), v,
                            preferred_element_type=jnp.float32)
                ctx_ref[:, h * DH:(h + 1) * DH] = (o / l).astype(jnp.bfloat16)

            @pl.when(u == 0)
            def _():
                w_loads[3].wait()
                wo_ref[...] = wf_ref[3].astype(jnp.bfloat16)

            part = jnp.dot(ctx_ref[...], wo_ref[...],
                           preferred_element_type=jnp.float32)

            @pl.when(u == 0)
            def _():
                out_ref[0] = part

            @pl.when(u == N_UNITS - 1)
            def _():
                out_ref[1] = part

            @pl.when(is_remote)
            def _():
                psend_ref[u] = part.astype(jnp.bfloat16)
                dev = jnp.where(u >= 5, diag, jnp.where(u % 2 == 1, left, right))
                pltpu.make_async_remote_copy(
                    src_ref=psend_ref.at[u], dst_ref=precv_ref.at[u],
                    send_sem=psend_sems.at[u], recv_sem=precv_sems.at[u],
                    device_id=(dev,), device_id_type=pl.DeviceIdType.MESH,
                ).start()

            return carry

        lax.fori_loop(0, N_UNITS, unit, 0)

        for r in x_rdmas:
            r.wait_send()
        for u in range(1, N_UNITS - 1):
            pltpu.make_async_remote_copy(
                src_ref=psend_ref.at[u], dst_ref=precv_ref.at[u],
                send_sem=psend_sems.at[u], recv_sem=precv_sems.at[u],
                device_id=(me,), device_id_type=pl.DeviceIdType.MESH,
            ).wait()

        out_ref[0] = (out_ref[0]
                      + precv_ref[1].astype(jnp.float32)
                      + precv_ref[2].astype(jnp.float32)
                      + precv_ref[5].astype(jnp.float32))
        out_ref[1] = (out_ref[1]
                      + precv_ref[3].astype(jnp.float32)
                      + precv_ref[4].astype(jnp.float32)
                      + precv_ref[6].astype(jnp.float32))

    out_shape = jax.ShapeDtypeStruct((B_LOC, SQ, D), jnp.float32)
    return pl.pallas_call(
        body,
        out_shape=out_shape,
        in_specs=[pl.BlockSpec(memory_space=pl.ANY)] * 5
        + [pl.BlockSpec(memory_space=pltpu.VMEM)] * 2,
        out_specs=pl.BlockSpec(memory_space=pltpu.VMEM),
        scratch_shapes=[
            pltpu.VMEM((B_LOC, SQ, D), jnp.float32),
            pltpu.VMEM((4, D, D), jnp.float32),
            pltpu.VMEM((3, D, D), jnp.bfloat16),
            pltpu.VMEM((D, D), jnp.bfloat16),
            pltpu.VMEM((N_UNITS, SQ, D), jnp.bfloat16),
            pltpu.VMEM((N_UNITS, SQ, D), jnp.bfloat16),
            pltpu.VMEM((N_UNITS, SQ, D), jnp.bfloat16),
            pltpu.VMEM((3 * H_LOC, SQ, DH), jnp.bfloat16),
            pltpu.VMEM((SQ, D), jnp.bfloat16),
            pltpu.SemaphoreType.DMA((6,)),
            pltpu.SemaphoreType.DMA((6,)),
            pltpu.SemaphoreType.DMA((N_UNITS,)),
            pltpu.SemaphoreType.DMA((N_UNITS,)),
            pltpu.SemaphoreType.DMA((N_UNITS,)),
        ],
        compiler_params=pltpu.CompilerParams(
            vmem_limit_bytes=100 * 1024 * 1024,
        ),
    )(x, Wq, Wk, Wv, Wo, jnp.asarray(cos_np), jnp.asarray(sin_np))
```

```python
import numpy as np

import jax
import jax.numpy as jnp
from jax import lax
from jax.experimental import pallas as pl
from jax.experimental.pallas import tpu as pltpu

N_DEV = 4
B_LOC = 2
SQ = 512
D = 1024
H_LOC = 8
DH = 128
N_UNITS = N_DEV * B_LOC
SCALE = 0.08838834764831843


def _rope_tables():
    inv = 1.0 / (10000.0 ** (np.arange(0, DH, 2) / DH))
    pos = np.arange(SQ)[:, None] * inv[None, :]
    cos = np.repeat(np.cos(pos), 2, axis=-1).astype(np.float32)
    sin = np.repeat(np.sin(pos), 2, axis=-1).astype(np.float32)
    sign = np.where(np.arange(DH) % 2 == 0, -1.0, 1.0).astype(np.float32)
    return cos, sin * sign[None, :]


def pallas_dist_rope_attn_htp_bs_b2_sq512_d1024_hq8_dh128_kernel(
    x: jax.Array,
    Wq: jax.Array,
    Wk: jax.Array,
    Wv: jax.Array,
    Wo: jax.Array,
):
    cos_np, sin_np = _rope_tables()

    def body(x_hbm, wq_hbm, wk_hbm, wv_hbm, wo_hbm, cos_ref, sin_ref, out_hbm,
             out_ref, xf_ref, wf_ref, wqkv_ref, wo_ref, xg_ref, psend_ref, precv_ref,
             qkv_ref, ctx_ref,
             load_sems, store_sems, xsend_sems, xrecv_sems, psend_sems, precv_sems):
        me = lax.axis_index("i")
        left = (me + N_DEV - 1) % N_DEV
        right = (me + 1) % N_DEV
        diag = (me + 2) % N_DEV

        x_loads = []
        for b in range(B_LOC):
            cp = pltpu.make_async_copy(x_hbm.at[b], xf_ref.at[b], load_sems.at[b])
            cp.start()
            x_loads.append(cp)
        w_loads = []
        for i, w in enumerate((wq_hbm, wk_hbm, wv_hbm, wo_hbm)):
            cp = pltpu.make_async_copy(w, wf_ref.at[i], load_sems.at[2 + i])
            cp.start()
            w_loads.append(cp)

        x_loads[0].wait()
        xg_ref[0] = xf_ref[0].astype(jnp.bfloat16)
        x_loads[1].wait()
        xg_ref[N_UNITS - 1] = xf_ref[1].astype(jnp.bfloat16)

        x_sends = [
            (0, 1, right), (0, 2, left),
            (N_UNITS - 1, 3, right), (N_UNITS - 1, 4, left),
            (0, 5, diag), (N_UNITS - 1, 6, diag),
        ]
        x_rdmas = []
        for i, (su, du, dev) in enumerate(x_sends):
            r = pltpu.make_async_remote_copy(
                src_ref=xg_ref.at[su], dst_ref=xg_ref.at[du],
                send_sem=xsend_sems.at[i], recv_sem=xrecv_sems.at[du],
                device_id=(dev,), device_id_type=pl.DeviceIdType.MESH)
            r.start()
            x_rdmas.append(r)

        lane = lax.broadcasted_iota(jnp.int32, (SQ, DH), 1)
        even = (lane % 2) == 0

        def unit(u, carry):
            is_remote = jnp.logical_and(u >= 1, u <= N_UNITS - 2)

            @pl.when(is_remote)
            def _():
                pltpu.make_async_remote_copy(
                    src_ref=xg_ref.at[u], dst_ref=xg_ref.at[u],
                    send_sem=xsend_sems.at[0], recv_sem=xrecv_sems.at[u],
                    device_id=(me,), device_id_type=pl.DeviceIdType.MESH,
                ).wait_recv()

            xu = xg_ref[u]
            cos = cos_ref[...]
            sin = sin_ref[...]
            for i in range(3):
                @pl.when(u == 0)
                def _():
                    w_loads[i].wait()
                    wqkv_ref[i] = wf_ref[i].astype(jnp.bfloat16)

                y = jnp.dot(xu, wqkv_ref[i], preferred_element_type=jnp.float32)
                for c in range(H_LOC):
                    t = y[:, c * DH:(c + 1) * DH]
                    if i < 2:
                        tr = jnp.where(even, pltpu.roll(t, DH - 1, 1),
                                       pltpu.roll(t, 1, 1))
                        t = t * cos + tr * sin
                    if i == 0:
                        t = t * SCALE
                    qkv_ref[i * H_LOC + c] = t.astype(jnp.bfloat16)

            for h in range(H_LOC):
                q = qkv_ref[h]
                k = qkv_ref[H_LOC + h]
                v = qkv_ref[2 * H_LOC + h]
                s = lax.dot_general(q, k, (((1,), (1,)), ((), ())),
                                    preferred_element_type=jnp.float32)
                m = jnp.max(s, axis=-1, keepdims=True)
                p = jnp.exp(s - m)
                l = jnp.sum(p, axis=-1, keepdims=True)
                o = jnp.dot(p.astype(jnp.bfloat16), v,
                            preferred_element_type=jnp.float32)
                ctx_ref[:, h * DH:(h + 1) * DH] = (o / l).astype(jnp.bfloat16)

            @pl.when(u == 0)
            def _():
                w_loads[3].wait()
                wo_ref[...] = wf_ref[3].astype(jnp.bfloat16)

            part = jnp.dot(ctx_ref[...], wo_ref[...],
                           preferred_element_type=jnp.float32)

            @pl.when(u == 0)
            def _():
                out_ref[0] = part

            @pl.when(u == N_UNITS - 1)
            def _():
                out_ref[1] = part

            @pl.when(u == N_UNITS - 2)
            def _():
                for j in (1, 2, 5):
                    pltpu.make_async_remote_copy(
                        src_ref=psend_ref.at[j], dst_ref=precv_ref.at[j],
                        send_sem=psend_sems.at[j], recv_sem=precv_sems.at[j],
                        device_id=(me,), device_id_type=pl.DeviceIdType.MESH,
                    ).wait_recv()
                out_ref[0] = (out_ref[0]
                              + precv_ref[1].astype(jnp.float32)
                              + precv_ref[2].astype(jnp.float32)
                              + precv_ref[5].astype(jnp.float32))
                pltpu.make_async_copy(out_ref.at[0], out_hbm.at[0],
                                      store_sems.at[0]).start()

            @pl.when(is_remote)
            def _():
                psend_ref[u] = part.astype(jnp.bfloat16)
                dev = jnp.where(u >= 5, diag, jnp.where(u % 2 == 1, left, right))
                pltpu.make_async_remote_copy(
                    src_ref=psend_ref.at[u], dst_ref=precv_ref.at[u],
                    send_sem=psend_sems.at[u], recv_sem=precv_sems.at[u],
                    device_id=(dev,), device_id_type=pl.DeviceIdType.MESH,
                ).start()

            return carry

        lax.fori_loop(0, N_UNITS, unit, 0)

        for r in x_rdmas:
            r.wait_send()
        for j in (3, 4, 6):
            pltpu.make_async_remote_copy(
                src_ref=psend_ref.at[j], dst_ref=precv_ref.at[j],
                send_sem=psend_sems.at[j], recv_sem=precv_sems.at[j],
                device_id=(me,), device_id_type=pl.DeviceIdType.MESH,
            ).wait_recv()
        out_ref[1] = (out_ref[1]
                      + precv_ref[3].astype(jnp.float32)
                      + precv_ref[4].astype(jnp.float32)
                      + precv_ref[6].astype(jnp.float32))
        st1 = pltpu.make_async_copy(out_ref.at[1], out_hbm.at[1], store_sems.at[1])
        st1.start()
        for u in range(1, N_UNITS - 1):
            pltpu.make_async_remote_copy(
                src_ref=psend_ref.at[u], dst_ref=precv_ref.at[u],
                send_sem=psend_sems.at[u], recv_sem=precv_sems.at[u],
                device_id=(me,), device_id_type=pl.DeviceIdType.MESH,
            ).wait_send()
        pltpu.make_async_copy(out_ref.at[0], out_hbm.at[0], store_sems.at[0]).wait()
        st1.wait()

    out_shape = jax.ShapeDtypeStruct((B_LOC, SQ, D), jnp.float32)
    return pl.pallas_call(
        body,
        out_shape=out_shape,
        in_specs=[pl.BlockSpec(memory_space=pl.ANY)] * 5
        + [pl.BlockSpec(memory_space=pltpu.VMEM)] * 2,
        out_specs=pl.BlockSpec(memory_space=pl.ANY),
        scratch_shapes=[
            pltpu.VMEM((B_LOC, SQ, D), jnp.float32),
            pltpu.VMEM((B_LOC, SQ, D), jnp.float32),
            pltpu.VMEM((4, D, D), jnp.float32),
            pltpu.VMEM((3, D, D), jnp.bfloat16),
            pltpu.VMEM((D, D), jnp.bfloat16),
            pltpu.VMEM((N_UNITS, SQ, D), jnp.bfloat16),
            pltpu.VMEM((N_UNITS, SQ, D), jnp.bfloat16),
            pltpu.VMEM((N_UNITS, SQ, D), jnp.bfloat16),
            pltpu.VMEM((3 * H_LOC, SQ, DH), jnp.bfloat16),
            pltpu.VMEM((SQ, D), jnp.bfloat16),
            pltpu.SemaphoreType.DMA((6,)),
            pltpu.SemaphoreType.DMA((2,)),
            pltpu.SemaphoreType.DMA((6,)),
            pltpu.SemaphoreType.DMA((N_UNITS,)),
            pltpu.SemaphoreType.DMA((N_UNITS,)),
            pltpu.SemaphoreType.DMA((N_UNITS,)),
        ],
        compiler_params=pltpu.CompilerParams(
            vmem_limit_bytes=100 * 1024 * 1024,
        ),
    )(x, Wq, Wk, Wv, Wo, jnp.asarray(cos_np), jnp.asarray(sin_np))
```

```python
import numpy as np

import jax
import jax.numpy as jnp
from jax import lax
from jax.experimental import pallas as pl
from jax.experimental.pallas import tpu as pltpu

N_DEV = 4
B_LOC = 2
SQ = 512
D = 1024
H_LOC = 8
DH = 128
N_UNITS = N_DEV * B_LOC
SCALE = 0.08838834764831843


def _rope_tables():
    inv = 1.0 / (10000.0 ** (np.arange(0, DH, 2) / DH))
    pos = np.arange(SQ)[:, None] * inv[None, :]
    cos = np.repeat(np.cos(pos), 2, axis=-1).astype(np.float32)
    sin = np.repeat(np.sin(pos), 2, axis=-1).astype(np.float32)
    sign = np.where(np.arange(DH) % 2 == 0, -1.0, 1.0).astype(np.float32)
    return cos, sin * sign[None, :]


def pallas_dist_rope_attn_htp_bs_b2_sq512_d1024_hq8_dh128_kernel(
    x: jax.Array,
    Wq: jax.Array,
    Wk: jax.Array,
    Wv: jax.Array,
    Wo: jax.Array,
):
    cos_np, sin_np = _rope_tables()

    def body(x_hbm, wq_hbm, wk_hbm, wv_hbm, wo_hbm, cos_ref, sin_ref, out_ref,
             xf_ref, wf_ref, wqkv_ref, wo_ref, xg_ref, psend_ref, precv_ref,
             qkv_ref, ctx_ref,
             load_sems, xsend_sems, xrecv_sems, psend_sems, precv_sems):
        me = lax.axis_index("i")
        left = (me + N_DEV - 1) % N_DEV
        right = (me + 1) % N_DEV
        diag = (me + 2) % N_DEV

        x_loads = []
        for b in range(B_LOC):
            cp = pltpu.make_async_copy(x_hbm.at[b], xf_ref.at[b], load_sems.at[b])
            cp.start()
            x_loads.append(cp)
        w_loads = []
        for i, w in enumerate((wq_hbm, wk_hbm, wv_hbm, wo_hbm)):
            cp = pltpu.make_async_copy(w, wf_ref.at[i], load_sems.at[2 + i])
            cp.start()
            w_loads.append(cp)

        x_loads[0].wait()
        xg_ref[0] = xf_ref[0].astype(jnp.bfloat16)
        x_loads[1].wait()
        xg_ref[N_UNITS - 1] = xf_ref[1].astype(jnp.bfloat16)

        x_sends = [
            (0, 1, right), (0, 2, left),
            (N_UNITS - 1, 3, right), (N_UNITS - 1, 4, left),
            (0, 5, diag), (N_UNITS - 1, 6, diag),
        ]
        x_rdmas = []
        for i, (su, du, dev) in enumerate(x_sends):
            r = pltpu.make_async_remote_copy(
                src_ref=xg_ref.at[su], dst_ref=xg_ref.at[du],
                send_sem=xsend_sems.at[i], recv_sem=xrecv_sems.at[du],
                device_id=(dev,), device_id_type=pl.DeviceIdType.MESH)
            r.start()
            x_rdmas.append(r)

        lane = lax.broadcasted_iota(jnp.int32, (SQ, DH), 1)
        even = (lane % 2) == 0

        def unit(u, carry):
            is_remote = jnp.logical_and(u >= 1, u <= N_UNITS - 2)

            @pl.when(is_remote)
            def _():
                pltpu.make_async_remote_copy(
                    src_ref=xg_ref.at[u], dst_ref=xg_ref.at[u],
                    send_sem=xsend_sems.at[0], recv_sem=xrecv_sems.at[u],
                    device_id=(me,), device_id_type=pl.DeviceIdType.MESH,
                ).wait_recv()

            xu = xg_ref[u]
            cos = cos_ref[...]
            sin = sin_ref[...]
            for i in range(3):
                @pl.when(u == 0)
                def _():
                    w_loads[i].wait()
                    wqkv_ref[i] = wf_ref[i].astype(jnp.bfloat16)

                y = jnp.dot(xu, wqkv_ref[i], preferred_element_type=jnp.float32)
                for c in range(H_LOC):
                    t = y[:, c * DH:(c + 1) * DH]
                    if i < 2:
                        tr = jnp.where(even, pltpu.roll(t, DH - 1, 1),
                                       pltpu.roll(t, 1, 1))
                        t = t * cos + tr * sin
                    if i == 0:
                        t = t * SCALE
                    qkv_ref[i * H_LOC + c] = t.astype(jnp.bfloat16)

            for h in range(H_LOC):
                q = qkv_ref[h]
                k = qkv_ref[H_LOC + h]
                v = qkv_ref[2 * H_LOC + h]
                s = lax.dot_general(q, k, (((1,), (1,)), ((), ())),
                                    preferred_element_type=jnp.float32)
                m = jnp.max(s, axis=-1, keepdims=True)
                p = jnp.exp(s - m)
                l = jnp.sum(p, axis=-1, keepdims=True)
                o = jnp.dot(p.astype(jnp.bfloat16), v,
                            preferred_element_type=jnp.float32)
                ctx_ref[:, h * DH:(h + 1) * DH] = (o / l).astype(jnp.bfloat16)

            @pl.when(u == 0)
            def _():
                w_loads[3].wait()
                wo_ref[...] = wf_ref[3].astype(jnp.bfloat16)

            part = jnp.dot(ctx_ref[...], wo_ref[...],
                           preferred_element_type=jnp.float32)

            @pl.when(u == 0)
            def _():
                out_ref[0] = part

            @pl.when(u == N_UNITS - 1)
            def _():
                out_ref[1] = part

            @pl.when(u == N_UNITS - 2)
            def _():
                for j in (1, 2, 5):
                    pltpu.make_async_remote_copy(
                        src_ref=psend_ref.at[j], dst_ref=precv_ref.at[j],
                        send_sem=psend_sems.at[j], recv_sem=precv_sems.at[j],
                        device_id=(me,), device_id_type=pl.DeviceIdType.MESH,
                    ).wait_recv()
                out_ref[0] = (out_ref[0]
                              + precv_ref[1].astype(jnp.float32)
                              + precv_ref[2].astype(jnp.float32)
                              + precv_ref[5].astype(jnp.float32))

            @pl.when(is_remote)
            def _():
                psend_ref[u] = part.astype(jnp.bfloat16)
                dev = jnp.where(u >= 5, diag, jnp.where(u % 2 == 1, left, right))
                pltpu.make_async_remote_copy(
                    src_ref=psend_ref.at[u], dst_ref=precv_ref.at[u],
                    send_sem=psend_sems.at[u], recv_sem=precv_sems.at[u],
                    device_id=(dev,), device_id_type=pl.DeviceIdType.MESH,
                ).start()

            return carry

        lax.fori_loop(0, N_UNITS, unit, 0)

        for r in x_rdmas:
            r.wait_send()
        for j in (3, 4, 6):
            pltpu.make_async_remote_copy(
                src_ref=psend_ref.at[j], dst_ref=precv_ref.at[j],
                send_sem=psend_sems.at[j], recv_sem=precv_sems.at[j],
                device_id=(me,), device_id_type=pl.DeviceIdType.MESH,
            ).wait_recv()
        out_ref[1] = (out_ref[1]
                      + precv_ref[3].astype(jnp.float32)
                      + precv_ref[4].astype(jnp.float32)
                      + precv_ref[6].astype(jnp.float32))
        for u in range(1, N_UNITS - 1):
            pltpu.make_async_remote_copy(
                src_ref=psend_ref.at[u], dst_ref=precv_ref.at[u],
                send_sem=psend_sems.at[u], recv_sem=precv_sems.at[u],
                device_id=(me,), device_id_type=pl.DeviceIdType.MESH,
            ).wait_send()

    out_shape = jax.ShapeDtypeStruct((B_LOC, SQ, D), jnp.float32)
    return pl.pallas_call(
        body,
        out_shape=out_shape,
        in_specs=[pl.BlockSpec(memory_space=pl.ANY)] * 5
        + [pl.BlockSpec(memory_space=pltpu.VMEM)] * 2,
        out_specs=pl.BlockSpec(memory_space=pltpu.VMEM),
        scratch_shapes=[
            pltpu.VMEM((B_LOC, SQ, D), jnp.float32),
            pltpu.VMEM((4, D, D), jnp.float32),
            pltpu.VMEM((3, D, D), jnp.bfloat16),
            pltpu.VMEM((D, D), jnp.bfloat16),
            pltpu.VMEM((N_UNITS, SQ, D), jnp.bfloat16),
            pltpu.VMEM((N_UNITS, SQ, D), jnp.bfloat16),
            pltpu.VMEM((N_UNITS, SQ, D), jnp.bfloat16),
            pltpu.VMEM((3 * H_LOC, SQ, DH), jnp.bfloat16),
            pltpu.VMEM((SQ, D), jnp.bfloat16),
            pltpu.SemaphoreType.DMA((6,)),
            pltpu.SemaphoreType.DMA((6,)),
            pltpu.SemaphoreType.DMA((N_UNITS,)),
            pltpu.SemaphoreType.DMA((N_UNITS,)),
            pltpu.SemaphoreType.DMA((N_UNITS,)),
        ],
        compiler_params=pltpu.CompilerParams(
            vmem_limit_bytes=100 * 1024 * 1024,
        ),
    )(x, Wq, Wk, Wv, Wo, jnp.asarray(cos_np), jnp.asarray(sin_np))
```

```python
import numpy as np

import jax
import jax.numpy as jnp
from jax import lax
from jax.experimental import pallas as pl
from jax.experimental.pallas import tpu as pltpu

N_DEV = 4
B_LOC = 2
SQ = 512
D = 1024
H_LOC = 8
DH = 128
N_UNITS = N_DEV * B_LOC
SCALE = 0.08838834764831843


def _rope_tables():
    inv = 1.0 / (10000.0 ** (np.arange(0, DH, 2) / DH))
    pos = np.arange(SQ)[:, None] * inv[None, :]
    cos = np.repeat(np.cos(pos), 2, axis=-1).astype(np.float32)
    sin = np.repeat(np.sin(pos), 2, axis=-1).astype(np.float32)
    sign = np.where(np.arange(DH) % 2 == 0, -1.0, 1.0).astype(np.float32)
    return cos, sin * sign[None, :]


def pallas_dist_rope_attn_htp_bs_b2_sq512_d1024_hq8_dh128_kernel(
    x: jax.Array,
    Wq: jax.Array,
    Wk: jax.Array,
    Wv: jax.Array,
    Wo: jax.Array,
):
    cos_np, sin_np = _rope_tables()

    def body(x_hbm, wq_hbm, wk_hbm, wv_hbm, wo_hbm, cos_ref, sin_ref, out_ref,
             xf_ref, wf_ref, wqkv_ref, wo_ref, xg_ref, psend_ref, precv_ref,
             qkv_ref, ctx_ref,
             load_sems, xsend_sems, xrecv_sems, psend_sems, precv_sems):
        me = lax.axis_index("i")
        left = (me + N_DEV - 1) % N_DEV
        right = (me + 1) % N_DEV
        diag = (me + 2) % N_DEV

        x_loads = [pltpu.make_async_copy(x_hbm.at[b], xf_ref.at[b], load_sems.at[b])
                   for b in range(B_LOC)]
        w_loads = [pltpu.make_async_copy(w, wf_ref.at[i], load_sems.at[2 + i])
                   for i, w in enumerate((wq_hbm, wk_hbm, wv_hbm, wo_hbm))]
        for cp in (x_loads[0], w_loads[0], x_loads[1], w_loads[1], w_loads[2],
                   w_loads[3]):
            cp.start()

        barrier_sem = pltpu.get_barrier_semaphore()
        for dev in (left, right, diag):
            pl.semaphore_signal(barrier_sem, inc=1, device_id=(dev,),
                                device_id_type=pl.DeviceIdType.MESH)
        pl.semaphore_wait(barrier_sem, 3)

        x_sends = [
            (0, 1, right), (0, 2, left), (0, 5, diag),
            (N_UNITS - 1, 3, right), (N_UNITS - 1, 4, left),
            (N_UNITS - 1, 6, diag),
        ]
        x_rdmas = [
            pltpu.make_async_remote_copy(
                src_ref=xg_ref.at[su], dst_ref=xg_ref.at[du],
                send_sem=xsend_sems.at[i], recv_sem=xrecv_sems.at[du],
                device_id=(dev,), device_id_type=pl.DeviceIdType.MESH)
            for i, (su, du, dev) in enumerate(x_sends)
        ]
        x_loads[0].wait()
        xg_ref[0] = xf_ref[0].astype(jnp.bfloat16)
        for r in x_rdmas[:3]:
            r.start()

        lane = lax.broadcasted_iota(jnp.int32, (SQ, DH), 1)
        even = (lane % 2) == 0

        def unit(u, carry):
            is_remote = jnp.logical_and(u >= 1, u <= N_UNITS - 2)

            @pl.when(is_remote)
            def _():
                pltpu.make_async_remote_copy(
                    src_ref=xg_ref.at[u], dst_ref=xg_ref.at[u],
                    send_sem=xsend_sems.at[0], recv_sem=xrecv_sems.at[u],
                    device_id=(me,), device_id_type=pl.DeviceIdType.MESH,
                ).wait_recv()

            xu = xg_ref[u]
            cos = cos_ref[...]
            sin = sin_ref[...]
            for i in range(3):
                @pl.when(u == 0)
                def _():
                    w_loads[i].wait()
                    wqkv_ref[i] = wf_ref[i].astype(jnp.bfloat16)

                if i == 1:
                    @pl.when(u == 0)
                    def _():
                        x_loads[1].wait()
                        xg_ref[N_UNITS - 1] = xf_ref[1].astype(jnp.bfloat16)
                        for r in x_rdmas[3:]:
                            r.start()

                y = jnp.dot(xu, wqkv_ref[i], preferred_element_type=jnp.float32)
                for c in range(H_LOC):
                    t = y[:, c * DH:(c + 1) * DH]
                    if i < 2:
                        tr = jnp.where(even, pltpu.roll(t, DH - 1, 1),
                                       pltpu.roll(t, 1, 1))
                        t = t * cos + tr * sin
                    if i == 0:
                        t = t * SCALE
                    qkv_ref[i * H_LOC + c] = t.astype(jnp.bfloat16)

            for h in range(H_LOC):
                q = qkv_ref[h]
                k = qkv_ref[H_LOC + h]
                v = qkv_ref[2 * H_LOC + h]
                s = lax.dot_general(q, k, (((1,), (1,)), ((), ())),
                                    preferred_element_type=jnp.float32)
                m = jnp.max(s, axis=-1, keepdims=True)
                p = jnp.exp(s - m)
                l = jnp.sum(p, axis=-1, keepdims=True)
                o = jnp.dot(p.astype(jnp.bfloat16), v,
                            preferred_element_type=jnp.float32)
                ctx_ref[:, h * DH:(h + 1) * DH] = (o / l).astype(jnp.bfloat16)

            @pl.when(u == 0)
            def _():
                w_loads[3].wait()
                wo_ref[...] = wf_ref[3].astype(jnp.bfloat16)

            part = jnp.dot(ctx_ref[...], wo_ref[...],
                           preferred_element_type=jnp.float32)

            @pl.when(u == 0)
            def _():
                out_ref[0] = part

            @pl.when(u == N_UNITS - 1)
            def _():
                out_ref[1] = part

            @pl.when(u == N_UNITS - 2)
            def _():
                for j in (1, 2, 5):
                    pltpu.make_async_remote_copy(
                        src_ref=psend_ref.at[j], dst_ref=precv_ref.at[j],
                        send_sem=psend_sems.at[j], recv_sem=precv_sems.at[j],
                        device_id=(me,), device_id_type=pl.DeviceIdType.MESH,
                    ).wait_recv()
                out_ref[0] = (out_ref[0]
                              + precv_ref[1].astype(jnp.float32)
                              + precv_ref[2].astype(jnp.float32)
                              + precv_ref[5].astype(jnp.float32))

            @pl.when(is_remote)
            def _():
                psend_ref[u] = part.astype(jnp.bfloat16)
                dev = jnp.where(u >= 5, diag, jnp.where(u % 2 == 1, left, right))
                pltpu.make_async_remote_copy(
                    src_ref=psend_ref.at[u], dst_ref=precv_ref.at[u],
                    send_sem=psend_sems.at[u], recv_sem=precv_sems.at[u],
                    device_id=(dev,), device_id_type=pl.DeviceIdType.MESH,
                ).start()

            return carry

        lax.fori_loop(0, N_UNITS, unit, 0)

        for r in x_rdmas:
            r.wait_send()
        for j in (3, 4, 6):
            pltpu.make_async_remote_copy(
                src_ref=psend_ref.at[j], dst_ref=precv_ref.at[j],
                send_sem=psend_sems.at[j], recv_sem=precv_sems.at[j],
                device_id=(me,), device_id_type=pl.DeviceIdType.MESH,
            ).wait_recv()
        out_ref[1] = (out_ref[1]
                      + precv_ref[3].astype(jnp.float32)
                      + precv_ref[4].astype(jnp.float32)
                      + precv_ref[6].astype(jnp.float32))
        for u in range(1, N_UNITS - 1):
            pltpu.make_async_remote_copy(
                src_ref=psend_ref.at[u], dst_ref=precv_ref.at[u],
                send_sem=psend_sems.at[u], recv_sem=precv_sems.at[u],
                device_id=(me,), device_id_type=pl.DeviceIdType.MESH,
            ).wait_send()

    out_shape = jax.ShapeDtypeStruct((B_LOC, SQ, D), jnp.float32)
    return pl.pallas_call(
        body,
        out_shape=out_shape,
        in_specs=[pl.BlockSpec(memory_space=pl.ANY)] * 5
        + [pl.BlockSpec(memory_space=pltpu.VMEM)] * 2,
        out_specs=pl.BlockSpec(memory_space=pltpu.VMEM),
        scratch_shapes=[
            pltpu.VMEM((B_LOC, SQ, D), jnp.float32),
            pltpu.VMEM((4, D, D), jnp.float32),
            pltpu.VMEM((3, D, D), jnp.bfloat16),
            pltpu.VMEM((D, D), jnp.bfloat16),
            pltpu.VMEM((N_UNITS, SQ, D), jnp.bfloat16),
            pltpu.VMEM((N_UNITS, SQ, D), jnp.bfloat16),
            pltpu.VMEM((N_UNITS, SQ, D), jnp.bfloat16),
            pltpu.VMEM((3 * H_LOC, SQ, DH), jnp.bfloat16),
            pltpu.VMEM((SQ, D), jnp.bfloat16),
            pltpu.SemaphoreType.DMA((6,)),
            pltpu.SemaphoreType.DMA((6,)),
            pltpu.SemaphoreType.DMA((N_UNITS,)),
            pltpu.SemaphoreType.DMA((N_UNITS,)),
            pltpu.SemaphoreType.DMA((N_UNITS,)),
        ],
        compiler_params=pltpu.CompilerParams(
            vmem_limit_bytes=100 * 1024 * 1024,
            collective_id=0,
        ),
    )(x, Wq, Wk, Wv, Wo, jnp.asarray(cos_np), jnp.asarray(sin_np))
```

```python
import numpy as np

import jax
import jax.numpy as jnp
from jax import lax
from jax.experimental import pallas as pl
from jax.experimental.pallas import tpu as pltpu

N_DEV = 4
B_LOC = 2
SQ = 512
D = 1024
H_LOC = 8
DH = 128
N_UNITS = N_DEV * B_LOC
SCALE = 0.08838834764831843
WC = 256
N_WC = D // WC


def _rope_tables():
    inv = 1.0 / (10000.0 ** (np.arange(0, DH, 2) / DH))
    pos = np.arange(SQ)[:, None] * inv[None, :]
    cos = np.repeat(np.cos(pos), 2, axis=-1).astype(np.float32)
    sin = np.repeat(np.sin(pos), 2, axis=-1).astype(np.float32)
    sign = np.where(np.arange(DH) % 2 == 0, -1.0, 1.0).astype(np.float32)
    return cos, sin * sign[None, :]


def pallas_dist_rope_attn_htp_bs_b2_sq512_d1024_hq8_dh128_kernel(
    x: jax.Array,
    Wq: jax.Array,
    Wk: jax.Array,
    Wv: jax.Array,
    Wo: jax.Array,
):
    cos_np, sin_np = _rope_tables()

    def body(x_hbm, wq_hbm, wk_hbm, wv_hbm, wo_hbm, cos_ref, sin_ref, out_ref,
             xf_ref, wf_ref, wof_ref, wqkv_ref, wo_ref, xg_ref, psend_ref, precv_ref,
             qkv_ref, ctx_ref,
             load_sems, xsend_sems, xrecv_sems, psend_sems, precv_sems):
        me = lax.axis_index("i")
        left = (me + N_DEV - 1) % N_DEV
        right = (me + 1) % N_DEV
        diag = (me + 2) % N_DEV

        x_loads = [pltpu.make_async_copy(x_hbm.at[b], xf_ref.at[b], load_sems.at[b])
                   for b in range(B_LOC)]
        w_loads = [
            [pltpu.make_async_copy(w.at[:, pl.ds(c * WC, WC)],
                                   wf_ref.at[:, pl.ds(i * D + c * WC, WC)],
                                   load_sems.at[2 + i * N_WC + c])
             for c in range(N_WC)]
            for i, w in enumerate((wq_hbm, wk_hbm, wv_hbm))]
        wo_load = pltpu.make_async_copy(wo_hbm, wof_ref, load_sems.at[2 + 3 * N_WC])
        x_loads[0].start()
        for i in range(3):
            for c in range(N_WC):
                w_loads[i][c].start()
        x_loads[1].start()
        wo_load.start()

        barrier_sem = pltpu.get_barrier_semaphore()
        for dev in (left, right, diag):
            pl.semaphore_signal(barrier_sem, inc=1, device_id=(dev,),
                                device_id_type=pl.DeviceIdType.MESH)
        pl.semaphore_wait(barrier_sem, 3)

        x_sends = [
            (0, 1, right), (0, 2, left), (0, 5, diag),
            (N_UNITS - 1, 3, right), (N_UNITS - 1, 4, left),
            (N_UNITS - 1, 6, diag),
        ]
        x_rdmas = [
            pltpu.make_async_remote_copy(
                src_ref=xg_ref.at[su], dst_ref=xg_ref.at[du],
                send_sem=xsend_sems.at[i], recv_sem=xrecv_sems.at[du],
                device_id=(dev,), device_id_type=pl.DeviceIdType.MESH)
            for i, (su, du, dev) in enumerate(x_sends)
        ]
        x_loads[0].wait()
        xg_ref[0] = xf_ref[0].astype(jnp.bfloat16)
        for r in x_rdmas[:3]:
            r.start()

        lane = lax.broadcasted_iota(jnp.int32, (SQ, DH), 1)
        even = (lane % 2) == 0

        def finish_head(y, c):
            if c < 2 * H_LOC:
                yr = jnp.where(even, pltpu.roll(y, DH - 1, 1), pltpu.roll(y, 1, 1))
                y = y * cos_ref[...] + yr * sin_ref[...]
            if c < H_LOC:
                y = y * SCALE
            qkv_ref[c] = y.astype(jnp.bfloat16)

        def attend_and_project():
            for h in range(H_LOC):
                q = qkv_ref[h]
                k = qkv_ref[H_LOC + h]
                v = qkv_ref[2 * H_LOC + h]
                s = lax.dot_general(q, k, (((1,), (1,)), ((), ())),
                                    preferred_element_type=jnp.float32)
                m = jnp.max(s, axis=-1, keepdims=True)
                p = jnp.exp(s - m)
                l = jnp.sum(p, axis=-1, keepdims=True)
                o = jnp.dot(p.astype(jnp.bfloat16), v,
                            preferred_element_type=jnp.float32)
                ctx_ref[:, h * DH:(h + 1) * DH] = (o / l).astype(jnp.bfloat16)
            return jnp.dot(ctx_ref[...], wo_ref[...],
                           preferred_element_type=jnp.float32)

        x0 = xg_ref[0]
        for i in range(3):
            for c in range(N_WC):
                w_loads[i][c].wait()
                cols = pl.ds(i * D + c * WC, WC)
                wb = wf_ref[:, cols].astype(jnp.bfloat16)
                wqkv_ref[:, cols] = wb
                y = jnp.dot(x0, wb, preferred_element_type=jnp.float32)
                for j in range(WC // DH):
                    finish_head(y[:, j * DH:(j + 1) * DH],
                                (i * D + c * WC) // DH + j)
        x_loads[1].wait()
        xg_ref[N_UNITS - 1] = xf_ref[1].astype(jnp.bfloat16)
        for r in x_rdmas[3:]:
            r.start()
        wo_load.wait()
        wo_ref[...] = wof_ref[...].astype(jnp.bfloat16)
        out_ref[0] = attend_and_project()

        def unit(u, carry):
            is_remote = u <= N_UNITS - 2

            @pl.when(is_remote)
            def _():
                pltpu.make_async_remote_copy(
                    src_ref=xg_ref.at[u], dst_ref=xg_ref.at[u],
                    send_sem=xsend_sems.at[0], recv_sem=xrecv_sems.at[u],
                    device_id=(me,), device_id_type=pl.DeviceIdType.MESH,
                ).wait_recv()

            y = jnp.dot(xg_ref[u], wqkv_ref[...],
                        preferred_element_type=jnp.float32)
            for c in range(3 * H_LOC):
                finish_head(y[:, c * DH:(c + 1) * DH], c)
            part = attend_and_project()

            @pl.when(u == N_UNITS - 1)
            def _():
                out_ref[1] = part

            @pl.when(is_remote)
            def _():
                psend_ref[u] = part.astype(jnp.bfloat16)
                dev = jnp.where(u >= 5, diag, jnp.where(u % 2 == 1, left, right))
                pltpu.make_async_remote_copy(
                    src_ref=psend_ref.at[u], dst_ref=precv_ref.at[u],
                    send_sem=psend_sems.at[u], recv_sem=precv_sems.at[u],
                    device_id=(dev,), device_id_type=pl.DeviceIdType.MESH,
                ).start()

            return carry

        lax.fori_loop(1, N_UNITS, unit, 0)

        for r in x_rdmas:
            r.wait_send()
        for j in range(1, N_UNITS - 1):
            pltpu.make_async_remote_copy(
                src_ref=psend_ref.at[j], dst_ref=precv_ref.at[j],
                send_sem=psend_sems.at[j], recv_sem=precv_sems.at[j],
                device_id=(me,), device_id_type=pl.DeviceIdType.MESH,
            ).wait_recv()
        out_ref[0] = (out_ref[0]
                      + precv_ref[1].astype(jnp.float32)
                      + precv_ref[2].astype(jnp.float32)
                      + precv_ref[5].astype(jnp.float32))
        out_ref[1] = (out_ref[1]
                      + precv_ref[3].astype(jnp.float32)
                      + precv_ref[4].astype(jnp.float32)
                      + precv_ref[6].astype(jnp.float32))
        for u in range(1, N_UNITS - 1):
            pltpu.make_async_remote_copy(
                src_ref=psend_ref.at[u], dst_ref=precv_ref.at[u],
                send_sem=psend_sems.at[u], recv_sem=precv_sems.at[u],
                device_id=(me,), device_id_type=pl.DeviceIdType.MESH,
            ).wait_send()

    out_shape = jax.ShapeDtypeStruct((B_LOC, SQ, D), jnp.float32)
    return pl.pallas_call(
        body,
        out_shape=out_shape,
        in_specs=[pl.BlockSpec(memory_space=pl.ANY)] * 5
        + [pl.BlockSpec(memory_space=pltpu.VMEM)] * 2,
        out_specs=pl.BlockSpec(memory_space=pltpu.VMEM),
        scratch_shapes=[
            pltpu.VMEM((B_LOC, SQ, D), jnp.float32),
            pltpu.VMEM((D, 3 * D), jnp.float32),
            pltpu.VMEM((D, D), jnp.float32),
            pltpu.VMEM((D, 3 * D), jnp.bfloat16),
            pltpu.VMEM((D, D), jnp.bfloat16),
            pltpu.VMEM((N_UNITS, SQ, D), jnp.bfloat16),
            pltpu.VMEM((N_UNITS, SQ, D), jnp.bfloat16),
            pltpu.VMEM((N_UNITS, SQ, D), jnp.bfloat16),
            pltpu.VMEM((3 * H_LOC, SQ, DH), jnp.bfloat16),
            pltpu.VMEM((SQ, D), jnp.bfloat16),
            pltpu.SemaphoreType.DMA((3 + 3 * N_WC,)),
            pltpu.SemaphoreType.DMA((6,)),
            pltpu.SemaphoreType.DMA((N_UNITS,)),
            pltpu.SemaphoreType.DMA((N_UNITS,)),
            pltpu.SemaphoreType.DMA((N_UNITS,)),
        ],
        compiler_params=pltpu.CompilerParams(
            vmem_limit_bytes=100 * 1024 * 1024,
            collective_id=0,
        ),
    )(x, Wq, Wk, Wv, Wo, jnp.asarray(cos_np), jnp.asarray(sin_np))
```

```python
import numpy as np

import jax
import jax.numpy as jnp
from jax import lax
from jax.experimental import pallas as pl
from jax.experimental.pallas import tpu as pltpu

N_DEV = 4
B_LOC = 2
SQ = 512
D = 1024
H_LOC = 8
DH = 128
N_UNITS = N_DEV * B_LOC
SCALE = 0.08838834764831843
WC = 256
N_WC = D // WC


def _rope_tables():
    inv = 1.0 / (10000.0 ** (np.arange(0, DH, 2) / DH))
    pos = np.arange(SQ)[:, None] * inv[None, :]
    cos = np.repeat(np.cos(pos), 2, axis=-1).astype(np.float32)
    sin = np.repeat(np.sin(pos), 2, axis=-1).astype(np.float32)
    sign = np.where(np.arange(DH) % 2 == 0, -1.0, 1.0).astype(np.float32)
    return cos, sin * sign[None, :]


def pallas_dist_rope_attn_htp_bs_b2_sq512_d1024_hq8_dh128_kernel(
    x: jax.Array,
    Wq: jax.Array,
    Wk: jax.Array,
    Wv: jax.Array,
    Wo: jax.Array,
):
    cos_np, sin_np = _rope_tables()

    def body(x_hbm, wq_hbm, wk_hbm, wv_hbm, wo_hbm, cos_ref, sin_ref, out_ref,
             xf_ref, wf_ref, wof_ref, wqkv_ref, wo_ref, xg_ref, psend_ref, precv_ref,
             qkv_ref, ctx_ref,
             load_sems, xsend_sems, xrecv_sems, psend_sems, precv_sems):
        me = lax.axis_index("i")
        left = (me + N_DEV - 1) % N_DEV
        right = (me + 1) % N_DEV
        diag = (me + 2) % N_DEV

        x_loads = [pltpu.make_async_copy(x_hbm.at[b], xf_ref.at[b], load_sems.at[b])
                   for b in range(B_LOC)]
        w_loads = [
            [pltpu.make_async_copy(w.at[pl.ds(c * WC, WC), :],
                                   wf_ref.at[i, pl.ds(c * WC, WC), :],
                                   load_sems.at[2 + i * N_WC + c])
             for c in range(N_WC)]
            for i, w in enumerate((wq_hbm, wk_hbm, wv_hbm))]
        wo_load = pltpu.make_async_copy(wo_hbm, wof_ref, load_sems.at[2 + 3 * N_WC])
        x_loads[0].start()
        for i in range(3):
            for c in range(N_WC):
                w_loads[i][c].start()
        x_loads[1].start()
        wo_load.start()

        barrier_sem = pltpu.get_barrier_semaphore()
        for dev in (left, right, diag):
            pl.semaphore_signal(barrier_sem, inc=1, device_id=(dev,),
                                device_id_type=pl.DeviceIdType.MESH)
        pl.semaphore_wait(barrier_sem, 3)

        x_sends = [
            (0, 1, right), (0, 2, left), (0, 5, diag),
            (N_UNITS - 1, 3, right), (N_UNITS - 1, 4, left),
            (N_UNITS - 1, 6, diag),
        ]
        x_rdmas = [
            pltpu.make_async_remote_copy(
                src_ref=xg_ref.at[su], dst_ref=xg_ref.at[du],
                send_sem=xsend_sems.at[i], recv_sem=xrecv_sems.at[du],
                device_id=(dev,), device_id_type=pl.DeviceIdType.MESH)
            for i, (su, du, dev) in enumerate(x_sends)
        ]
        x_loads[0].wait()
        xg_ref[0] = xf_ref[0].astype(jnp.bfloat16)
        for r in x_rdmas[:3]:
            r.start()

        lane = lax.broadcasted_iota(jnp.int32, (SQ, DH), 1)
        even = (lane % 2) == 0

        def finish_head(y, c):
            if c < 2 * H_LOC:
                yr = jnp.where(even, pltpu.roll(y, DH - 1, 1), pltpu.roll(y, 1, 1))
                y = y * cos_ref[...] + yr * sin_ref[...]
            if c < H_LOC:
                y = y * SCALE
            qkv_ref[c] = y.astype(jnp.bfloat16)

        def attend_and_project():
            for h in range(H_LOC):
                q = qkv_ref[h]
                k = qkv_ref[H_LOC + h]
                v = qkv_ref[2 * H_LOC + h]
                s = lax.dot_general(q, k, (((1,), (1,)), ((), ())),
                                    preferred_element_type=jnp.float32)
                m = jnp.max(s, axis=-1, keepdims=True)
                p = jnp.exp(s - m)
                l = jnp.sum(p, axis=-1, keepdims=True)
                o = jnp.dot(p.astype(jnp.bfloat16), v,
                            preferred_element_type=jnp.float32)
                ctx_ref[:, h * DH:(h + 1) * DH] = (o / l).astype(jnp.bfloat16)
            return jnp.dot(ctx_ref[...], wo_ref[...],
                           preferred_element_type=jnp.float32)

        for i in range(3):
            y = None
            for c in range(N_WC):
                w_loads[i][c].wait()
                rows = pl.ds(c * WC, WC)
                wb = wf_ref[i, rows, :].astype(jnp.bfloat16)
                wqkv_ref[rows, i * D:(i + 1) * D] = wb
                d = jnp.dot(xg_ref[0, :, c * WC:(c + 1) * WC], wb,
                            preferred_element_type=jnp.float32)
                y = d if y is None else y + d
            for j in range(H_LOC):
                finish_head(y[:, j * DH:(j + 1) * DH], i * H_LOC + j)
        x_loads[1].wait()
        xg_ref[N_UNITS - 1] = xf_ref[1].astype(jnp.bfloat16)
        for r in x_rdmas[3:]:
            r.start()
        wo_load.wait()
        wo_ref[...] = wof_ref[...].astype(jnp.bfloat16)
        out_ref[0] = attend_and_project()

        def unit(u, carry):
            is_remote = u <= N_UNITS - 2

            @pl.when(is_remote)
            def _():
                pltpu.make_async_remote_copy(
                    src_ref=xg_ref.at[u], dst_ref=xg_ref.at[u],
                    send_sem=xsend_sems.at[0], recv_sem=xrecv_sems.at[u],
                    device_id=(me,), device_id_type=pl.DeviceIdType.MESH,
                ).wait_recv()

            y = jnp.dot(xg_ref[u], wqkv_ref[...],
                        preferred_element_type=jnp.float32)
            for c in range(3 * H_LOC):
                finish_head(y[:, c * DH:(c + 1) * DH], c)
            part = attend_and_project()

            @pl.when(u == N_UNITS - 1)
            def _():
                out_ref[1] = part

            @pl.when(is_remote)
            def _():
                psend_ref[u] = part.astype(jnp.bfloat16)
                dev = jnp.where(u >= 5, diag, jnp.where(u % 2 == 1, left, right))
                pltpu.make_async_remote_copy(
                    src_ref=psend_ref.at[u], dst_ref=precv_ref.at[u],
                    send_sem=psend_sems.at[u], recv_sem=precv_sems.at[u],
                    device_id=(dev,), device_id_type=pl.DeviceIdType.MESH,
                ).start()

            return carry

        lax.fori_loop(1, N_UNITS, unit, 0)

        for r in x_rdmas:
            r.wait_send()
        for j in range(1, N_UNITS - 1):
            pltpu.make_async_remote_copy(
                src_ref=psend_ref.at[j], dst_ref=precv_ref.at[j],
                send_sem=psend_sems.at[j], recv_sem=precv_sems.at[j],
                device_id=(me,), device_id_type=pl.DeviceIdType.MESH,
            ).wait_recv()
        out_ref[0] = (out_ref[0]
                      + precv_ref[1].astype(jnp.float32)
                      + precv_ref[2].astype(jnp.float32)
                      + precv_ref[5].astype(jnp.float32))
        out_ref[1] = (out_ref[1]
                      + precv_ref[3].astype(jnp.float32)
                      + precv_ref[4].astype(jnp.float32)
                      + precv_ref[6].astype(jnp.float32))
        for u in range(1, N_UNITS - 1):
            pltpu.make_async_remote_copy(
                src_ref=psend_ref.at[u], dst_ref=precv_ref.at[u],
                send_sem=psend_sems.at[u], recv_sem=precv_sems.at[u],
                device_id=(me,), device_id_type=pl.DeviceIdType.MESH,
            ).wait_send()

    out_shape = jax.ShapeDtypeStruct((B_LOC, SQ, D), jnp.float32)
    return pl.pallas_call(
        body,
        out_shape=out_shape,
        in_specs=[pl.BlockSpec(memory_space=pl.ANY)] * 5
        + [pl.BlockSpec(memory_space=pltpu.VMEM)] * 2,
        out_specs=pl.BlockSpec(memory_space=pltpu.VMEM),
        scratch_shapes=[
            pltpu.VMEM((B_LOC, SQ, D), jnp.float32),
            pltpu.VMEM((3, D, D), jnp.float32),
            pltpu.VMEM((D, D), jnp.float32),
            pltpu.VMEM((D, 3 * D), jnp.bfloat16),
            pltpu.VMEM((D, D), jnp.bfloat16),
            pltpu.VMEM((N_UNITS, SQ, D), jnp.bfloat16),
            pltpu.VMEM((N_UNITS, SQ, D), jnp.bfloat16),
            pltpu.VMEM((N_UNITS, SQ, D), jnp.bfloat16),
            pltpu.VMEM((3 * H_LOC, SQ, DH), jnp.bfloat16),
            pltpu.VMEM((SQ, D), jnp.bfloat16),
            pltpu.SemaphoreType.DMA((3 + 3 * N_WC,)),
            pltpu.SemaphoreType.DMA((6,)),
            pltpu.SemaphoreType.DMA((N_UNITS,)),
            pltpu.SemaphoreType.DMA((N_UNITS,)),
            pltpu.SemaphoreType.DMA((N_UNITS,)),
        ],
        compiler_params=pltpu.CompilerParams(
            vmem_limit_bytes=100 * 1024 * 1024,
            collective_id=0,
        ),
    )(x, Wq, Wk, Wv, Wo, jnp.asarray(cos_np), jnp.asarray(sin_np))
```

```python
import numpy as np

import jax
import jax.numpy as jnp
from jax import lax
from jax.experimental import pallas as pl
from jax.experimental.pallas import tpu as pltpu

N_DEV = 4
B_LOC = 2
SQ = 512
D = 1024
H_LOC = 8
DH = 128
N_UNITS = N_DEV * B_LOC
SCALE = 0.08838834764831843
WC = 256
N_WC = D // WC


def _rope_tables():
    inv = 1.0 / (10000.0 ** (np.arange(0, DH, 2) / DH))
    pos = np.arange(SQ)[:, None] * inv[None, :]
    cos = np.repeat(np.cos(pos), 2, axis=-1).astype(np.float32)
    sin = np.repeat(np.sin(pos), 2, axis=-1).astype(np.float32)
    sign = np.where(np.arange(DH) % 2 == 0, -1.0, 1.0).astype(np.float32)
    return cos, sin * sign[None, :]


def pallas_dist_rope_attn_htp_bs_b2_sq512_d1024_hq8_dh128_kernel(
    x: jax.Array,
    Wq: jax.Array,
    Wk: jax.Array,
    Wv: jax.Array,
    Wo: jax.Array,
):
    cos_np, sin_np = _rope_tables()

    def body(x_hbm, wq_hbm, wk_hbm, wv_hbm, wo_hbm, cos_ref, sin_ref, out_ref,
             xf_ref, wf_ref, wof_ref, wqkv_ref, wo_ref, xg_ref, psend_ref, precv_ref,
             qkv_ref, ctx_ref,
             load_sems, xsend_sems, xrecv_sems, psend_sems, precv_sems):
        me = lax.axis_index("i")
        left = (me + N_DEV - 1) % N_DEV
        right = (me + 1) % N_DEV
        diag = (me + 2) % N_DEV

        x_loads = [pltpu.make_async_copy(x_hbm.at[b], xf_ref.at[b], load_sems.at[b])
                   for b in range(B_LOC)]
        w_loads = [
            [pltpu.make_async_copy(w.at[pl.ds(c * WC, WC), :],
                                   wf_ref.at[i, pl.ds(c * WC, WC), :],
                                   load_sems.at[2 + i * N_WC + c])
             for c in range(N_WC)]
            for i, w in enumerate((wq_hbm, wk_hbm, wv_hbm))]
        wo_load = pltpu.make_async_copy(wo_hbm, wof_ref, load_sems.at[2 + 3 * N_WC])
        x_loads[0].start()
        for i in range(3):
            for c in range(N_WC):
                w_loads[i][c].start()
        x_loads[1].start()
        wo_load.start()

        barrier_sem = pltpu.get_barrier_semaphore()
        for dev in (left, right, diag):
            pl.semaphore_signal(barrier_sem, inc=1, device_id=(dev,),
                                device_id_type=pl.DeviceIdType.MESH)
        pl.semaphore_wait(barrier_sem, 3)

        x_sends = [
            (0, 1, right), (0, 2, left), (0, 5, diag),
            (N_UNITS - 1, 3, right), (N_UNITS - 1, 4, left),
            (N_UNITS - 1, 6, diag),
        ]
        x_rdmas = [
            pltpu.make_async_remote_copy(
                src_ref=xg_ref.at[su], dst_ref=xg_ref.at[du],
                send_sem=xsend_sems.at[i], recv_sem=xrecv_sems.at[du],
                device_id=(dev,), device_id_type=pl.DeviceIdType.MESH)
            for i, (su, du, dev) in enumerate(x_sends)
        ]
        x_loads[0].wait()
        xg_ref[0] = xf_ref[0].astype(jnp.bfloat16)
        for r in x_rdmas[:3]:
            r.start()

        lane = lax.broadcasted_iota(jnp.int32, (SQ, DH), 1)
        even = (lane % 2) == 0

        def finish_head(y, c):
            if c < 2 * H_LOC:
                yr = jnp.where(even, pltpu.roll(y, DH - 1, 1), pltpu.roll(y, 1, 1))
                y = y * cos_ref[...] + yr * sin_ref[...]
            if c < H_LOC:
                y = y * SCALE
            qkv_ref[c] = y.astype(jnp.bfloat16)

        def attend_and_project(first=False):
            for h in range(H_LOC):
                q = qkv_ref[h]
                k = qkv_ref[H_LOC + h]
                v = qkv_ref[2 * H_LOC + h]
                s = lax.dot_general(q, k, (((1,), (1,)), ((), ())),
                                    preferred_element_type=jnp.float32)
                m = jnp.max(s, axis=-1, keepdims=True)
                p = jnp.exp(s - m)
                l = jnp.sum(p, axis=-1, keepdims=True)
                o = jnp.dot(p.astype(jnp.bfloat16), v,
                            preferred_element_type=jnp.float32)
                ctx_ref[:, h * DH:(h + 1) * DH] = (o / l).astype(jnp.bfloat16)
            if first:
                wo_load.wait()
                wo_ref[...] = wof_ref[...].astype(jnp.bfloat16)
            return jnp.dot(ctx_ref[...], wo_ref[...],
                           preferred_element_type=jnp.float32)

        for i in range(3):
            y = None
            for c in range(N_WC):
                w_loads[i][c].wait()
                rows = pl.ds(c * WC, WC)
                wb = wf_ref[i, rows, :].astype(jnp.bfloat16)
                wqkv_ref[rows, i * D:(i + 1) * D] = wb
                d = jnp.dot(xg_ref[0, :, c * WC:(c + 1) * WC], wb,
                            preferred_element_type=jnp.float32)
                y = d if y is None else y + d
            for j in range(H_LOC):
                finish_head(y[:, j * DH:(j + 1) * DH], i * H_LOC + j)
        x_loads[1].wait()
        xg_ref[N_UNITS - 1] = xf_ref[1].astype(jnp.bfloat16)
        for r in x_rdmas[3:]:
            r.start()
        out_ref[0] = attend_and_project(first=True)

        def unit(u, carry):
            is_remote = u <= N_UNITS - 2

            @pl.when(is_remote)
            def _():
                pltpu.make_async_remote_copy(
                    src_ref=xg_ref.at[u], dst_ref=xg_ref.at[u],
                    send_sem=xsend_sems.at[0], recv_sem=xrecv_sems.at[u],
                    device_id=(me,), device_id_type=pl.DeviceIdType.MESH,
                ).wait_recv()

            y = jnp.dot(xg_ref[u], wqkv_ref[...],
                        preferred_element_type=jnp.float32)
            for c in range(3 * H_LOC):
                finish_head(y[:, c * DH:(c + 1) * DH], c)
            part = attend_and_project()

            @pl.when(u == N_UNITS - 1)
            def _():
                out_ref[1] = part

            @pl.when(is_remote)
            def _():
                psend_ref[u] = part.astype(jnp.bfloat16)
                dev = jnp.where(u >= 5, diag, jnp.where(u % 2 == 1, left, right))
                pltpu.make_async_remote_copy(
                    src_ref=psend_ref.at[u], dst_ref=precv_ref.at[u],
                    send_sem=psend_sems.at[u], recv_sem=precv_sems.at[u],
                    device_id=(dev,), device_id_type=pl.DeviceIdType.MESH,
                ).start()

            return carry

        lax.fori_loop(1, N_UNITS, unit, 0)

        for r in x_rdmas:
            r.wait_send()
        for j in range(1, N_UNITS - 1):
            pltpu.make_async_remote_copy(
                src_ref=psend_ref.at[j], dst_ref=precv_ref.at[j],
                send_sem=psend_sems.at[j], recv_sem=precv_sems.at[j],
                device_id=(me,), device_id_type=pl.DeviceIdType.MESH,
            ).wait_recv()
        out_ref[0] = (out_ref[0]
                      + precv_ref[1].astype(jnp.float32)
                      + precv_ref[2].astype(jnp.float32)
                      + precv_ref[5].astype(jnp.float32))
        out_ref[1] = (out_ref[1]
                      + precv_ref[3].astype(jnp.float32)
                      + precv_ref[4].astype(jnp.float32)
                      + precv_ref[6].astype(jnp.float32))
        for u in range(1, N_UNITS - 1):
            pltpu.make_async_remote_copy(
                src_ref=psend_ref.at[u], dst_ref=precv_ref.at[u],
                send_sem=psend_sems.at[u], recv_sem=precv_sems.at[u],
                device_id=(me,), device_id_type=pl.DeviceIdType.MESH,
            ).wait_send()

    out_shape = jax.ShapeDtypeStruct((B_LOC, SQ, D), jnp.float32)
    return pl.pallas_call(
        body,
        out_shape=out_shape,
        in_specs=[pl.BlockSpec(memory_space=pl.ANY)] * 5
        + [pl.BlockSpec(memory_space=pltpu.VMEM)] * 2,
        out_specs=pl.BlockSpec(memory_space=pltpu.VMEM),
        scratch_shapes=[
            pltpu.VMEM((B_LOC, SQ, D), jnp.float32),
            pltpu.VMEM((3, D, D), jnp.float32),
            pltpu.VMEM((D, D), jnp.float32),
            pltpu.VMEM((D, 3 * D), jnp.bfloat16),
            pltpu.VMEM((D, D), jnp.bfloat16),
            pltpu.VMEM((N_UNITS, SQ, D), jnp.bfloat16),
            pltpu.VMEM((N_UNITS, SQ, D), jnp.bfloat16),
            pltpu.VMEM((N_UNITS, SQ, D), jnp.bfloat16),
            pltpu.VMEM((3 * H_LOC, SQ, DH), jnp.bfloat16),
            pltpu.VMEM((SQ, D), jnp.bfloat16),
            pltpu.SemaphoreType.DMA((3 + 3 * N_WC,)),
            pltpu.SemaphoreType.DMA((6,)),
            pltpu.SemaphoreType.DMA((N_UNITS,)),
            pltpu.SemaphoreType.DMA((N_UNITS,)),
            pltpu.SemaphoreType.DMA((N_UNITS,)),
        ],
        compiler_params=pltpu.CompilerParams(
            vmem_limit_bytes=100 * 1024 * 1024,
            collective_id=0,
        ),
    )(x, Wq, Wk, Wv, Wo, jnp.asarray(cos_np), jnp.asarray(sin_np))
```

```python
import numpy as np

import jax
import jax.numpy as jnp
from jax import lax
from jax.experimental import pallas as pl
from jax.experimental.pallas import tpu as pltpu

N_DEV = 4
B_LOC = 2
SQ = 512
D = 1024
H_LOC = 8
DH = 128
N_UNITS = N_DEV * B_LOC
SCALE = 0.08838834764831843
WC = 256
N_WC = D // WC


def _rope_tables():
    inv = 1.0 / (10000.0 ** (np.arange(0, DH, 2) / DH))
    pos = np.arange(SQ)[:, None] * inv[None, :]
    cos = np.repeat(np.cos(pos), 2, axis=-1).astype(np.float32)
    sin = np.repeat(np.sin(pos), 2, axis=-1).astype(np.float32)
    sign = np.where(np.arange(DH) % 2 == 0, -1.0, 1.0).astype(np.float32)
    return cos, sin * sign[None, :]


def pallas_dist_rope_attn_htp_bs_b2_sq512_d1024_hq8_dh128_kernel(
    x: jax.Array,
    Wq: jax.Array,
    Wk: jax.Array,
    Wv: jax.Array,
    Wo: jax.Array,
):
    cos_np, sin_np = _rope_tables()

    def body(x_hbm, wq_hbm, wk_hbm, wv_hbm, wo_hbm, cos_ref, sin_ref, out_ref,
             xf_ref, wf_ref, wof_ref, wqkv_ref, wo_ref, xg_ref, psend_ref, precv_ref,
             qkv_ref, ctx_ref,
             load_sems, xsend_sems, xrecv_sems, psend_sems, precv_sems):
        me = lax.axis_index("i")
        left = (me + N_DEV - 1) % N_DEV
        right = (me + 1) % N_DEV
        diag = (me + 2) % N_DEV

        x_loads = [pltpu.make_async_copy(x_hbm.at[b], xf_ref.at[b], load_sems.at[b])
                   for b in range(B_LOC)]
        w_loads = [
            [pltpu.make_async_copy(w.at[pl.ds(c * WC, WC), :],
                                   wf_ref.at[i, pl.ds(c * WC, WC), :],
                                   load_sems.at[2 + i * N_WC + c])
             for c in range(N_WC)]
            for i, w in enumerate((wq_hbm, wk_hbm, wv_hbm))]
        wo_load = pltpu.make_async_copy(wo_hbm, wof_ref, load_sems.at[2 + 3 * N_WC])
        x_loads[0].start()
        for i in range(3):
            for c in range(N_WC):
                w_loads[i][c].start()
        x_loads[1].start()
        wo_load.start()

        barrier_sem = pltpu.get_barrier_semaphore()
        for dev in (left, right, diag):
            pl.semaphore_signal(barrier_sem, inc=1, device_id=(dev,),
                                device_id_type=pl.DeviceIdType.MESH)
        pl.semaphore_wait(barrier_sem, 3)

        x_sends = [
            (0, 1, right), (0, 2, left), (0, 5, diag),
            (N_UNITS - 1, 3, right), (N_UNITS - 1, 4, left),
            (N_UNITS - 1, 6, diag),
        ]
        x_rdmas = [
            pltpu.make_async_remote_copy(
                src_ref=xg_ref.at[su], dst_ref=xg_ref.at[du],
                send_sem=xsend_sems.at[i], recv_sem=xrecv_sems.at[du],
                device_id=(dev,), device_id_type=pl.DeviceIdType.MESH)
            for i, (su, du, dev) in enumerate(x_sends)
        ]
        x_loads[0].wait()
        xg_ref[0] = xf_ref[0].astype(jnp.bfloat16)
        for r in x_rdmas[:3]:
            r.start()

        lane = lax.broadcasted_iota(jnp.int32, (SQ, DH), 1)
        even = (lane % 2) == 0

        def finish_head(y, c):
            if c < 2 * H_LOC:
                yr = jnp.where(even, pltpu.roll(y, DH - 1, 1), pltpu.roll(y, 1, 1))
                y = y * cos_ref[...] + yr * sin_ref[...]
            if c < H_LOC:
                y = y * SCALE
            qkv_ref[c] = y.astype(jnp.bfloat16)

        def attend_head(h):
            q = qkv_ref[h]
            k = qkv_ref[H_LOC + h]
            v = qkv_ref[2 * H_LOC + h]
            s = lax.dot_general(q, k, (((1,), (1,)), ((), ())),
                                preferred_element_type=jnp.float32)
            m = jnp.max(s, axis=-1, keepdims=True)
            p = jnp.exp(s - m)
            l = jnp.sum(p, axis=-1, keepdims=True)
            o = jnp.dot(p.astype(jnp.bfloat16), v,
                        preferred_element_type=jnp.float32)
            return (o / l).astype(jnp.bfloat16)

        def attend_and_project():
            for h in range(H_LOC):
                ctx_ref[:, h * DH:(h + 1) * DH] = attend_head(h)
            return jnp.dot(ctx_ref[...], wo_ref[...],
                           preferred_element_type=jnp.float32)

        def proj0(i, carry):
            y = None
            for c in range(N_WC):
                rows = pl.ds(c * WC, WC)
                pltpu.make_async_copy(
                    wq_hbm.at[rows, :], wf_ref.at[i, rows, :],
                    load_sems.at[2 + i * N_WC + c]).wait()
                wb = wf_ref[i, rows, :].astype(jnp.bfloat16)
                wqkv_ref[rows, pl.ds(pl.multiple_of(i * D, DH), D)] = wb
                d = jnp.dot(xg_ref[0, :, c * WC:(c + 1) * WC], wb,
                            preferred_element_type=jnp.float32)
                y = d if y is None else y + d
            is_qk = i < 2
            mul = jnp.where(i == 0, SCALE, 1.0).astype(jnp.float32)
            cos_i = jnp.where(is_qk, cos_ref[...], 1.0) * mul
            sin_i = jnp.where(is_qk, sin_ref[...], 0.0) * mul
            for j in range(H_LOC):
                t = y[:, j * DH:(j + 1) * DH]
                tr = jnp.where(even, pltpu.roll(t, DH - 1, 1), pltpu.roll(t, 1, 1))
                qkv_ref[i * H_LOC + j] = (t * cos_i + tr * sin_i).astype(jnp.bfloat16)
            return carry

        lax.fori_loop(0, 3, proj0, 0)
        x_loads[1].wait()
        xg_ref[N_UNITS - 1] = xf_ref[1].astype(jnp.bfloat16)
        for r in x_rdmas[3:]:
            r.start()

        def head0(h, carry):
            ctx_ref[:, pl.ds(pl.multiple_of(h * DH, DH), DH)] = attend_head(h)
            return carry

        lax.fori_loop(0, H_LOC, head0, 0, unroll=2)
        wo_load.wait()
        wo_ref[...] = wof_ref[...].astype(jnp.bfloat16)

        def oproj0(c, carry):
            cols = pl.ds(pl.multiple_of(c * WC, WC), WC)
            out_ref[0, :, cols] = jnp.dot(ctx_ref[...], wo_ref[:, cols],
                                          preferred_element_type=jnp.float32)
            return carry

        lax.fori_loop(0, N_WC, oproj0, 0)

        def unit(u, carry):
            is_remote = u <= N_UNITS - 2

            @pl.when(is_remote)
            def _():
                pltpu.make_async_remote_copy(
                    src_ref=xg_ref.at[u], dst_ref=xg_ref.at[u],
                    send_sem=xsend_sems.at[0], recv_sem=xrecv_sems.at[u],
                    device_id=(me,), device_id_type=pl.DeviceIdType.MESH,
                ).wait_recv()

            y = jnp.dot(xg_ref[u], wqkv_ref[...],
                        preferred_element_type=jnp.float32)
            for c in range(3 * H_LOC):
                finish_head(y[:, c * DH:(c + 1) * DH], c)
            part = attend_and_project()

            @pl.when(u == N_UNITS - 1)
            def _():
                out_ref[1] = part

            @pl.when(is_remote)
            def _():
                psend_ref[u] = part.astype(jnp.bfloat16)
                dev = jnp.where(u >= 5, diag, jnp.where(u % 2 == 1, left, right))
                pltpu.make_async_remote_copy(
                    src_ref=psend_ref.at[u], dst_ref=precv_ref.at[u],
                    send_sem=psend_sems.at[u], recv_sem=precv_sems.at[u],
                    device_id=(dev,), device_id_type=pl.DeviceIdType.MESH,
                ).start()

            return carry

        lax.fori_loop(1, N_UNITS, unit, 0)

        for r in x_rdmas:
            r.wait_send()
        for j in range(1, N_UNITS - 1):
            pltpu.make_async_remote_copy(
                src_ref=psend_ref.at[j], dst_ref=precv_ref.at[j],
                send_sem=psend_sems.at[j], recv_sem=precv_sems.at[j],
                device_id=(me,), device_id_type=pl.DeviceIdType.MESH,
            ).wait_recv()
        out_ref[0] = (out_ref[0]
                      + precv_ref[1].astype(jnp.float32)
                      + precv_ref[2].astype(jnp.float32)
                      + precv_ref[5].astype(jnp.float32))
        out_ref[1] = (out_ref[1]
                      + precv_ref[3].astype(jnp.float32)
                      + precv_ref[4].astype(jnp.float32)
                      + precv_ref[6].astype(jnp.float32))
        for u in range(1, N_UNITS - 1):
            pltpu.make_async_remote_copy(
                src_ref=psend_ref.at[u], dst_ref=precv_ref.at[u],
                send_sem=psend_sems.at[u], recv_sem=precv_sems.at[u],
                device_id=(me,), device_id_type=pl.DeviceIdType.MESH,
            ).wait_send()

    out_shape = jax.ShapeDtypeStruct((B_LOC, SQ, D), jnp.float32)
    return pl.pallas_call(
        body,
        out_shape=out_shape,
        in_specs=[pl.BlockSpec(memory_space=pl.ANY)] * 5
        + [pl.BlockSpec(memory_space=pltpu.VMEM)] * 2,
        out_specs=pl.BlockSpec(memory_space=pltpu.VMEM),
        scratch_shapes=[
            pltpu.VMEM((B_LOC, SQ, D), jnp.float32),
            pltpu.VMEM((3, D, D), jnp.float32),
            pltpu.VMEM((D, D), jnp.float32),
            pltpu.VMEM((D, 3 * D), jnp.bfloat16),
            pltpu.VMEM((D, D), jnp.bfloat16),
            pltpu.VMEM((N_UNITS, SQ, D), jnp.bfloat16),
            pltpu.VMEM((N_UNITS, SQ, D), jnp.bfloat16),
            pltpu.VMEM((N_UNITS, SQ, D), jnp.bfloat16),
            pltpu.VMEM((3 * H_LOC, SQ, DH), jnp.bfloat16),
            pltpu.VMEM((SQ, D), jnp.bfloat16),
            pltpu.SemaphoreType.DMA((3 + 3 * N_WC,)),
            pltpu.SemaphoreType.DMA((6,)),
            pltpu.SemaphoreType.DMA((N_UNITS,)),
            pltpu.SemaphoreType.DMA((N_UNITS,)),
            pltpu.SemaphoreType.DMA((N_UNITS,)),
        ],
        compiler_params=pltpu.CompilerParams(
            vmem_limit_bytes=100 * 1024 * 1024,
            collective_id=0,
        ),
    )(x, Wq, Wk, Wv, Wo, jnp.asarray(cos_np), jnp.asarray(sin_np))
```
